```python
import numpy as np

kernel_name = "dist_sparse_attn_strided_htp_bs_b2_sq256_skv256_hq4_dh64"

def setup_inputs():
    x = np.random.randn(8, 256, 512).astype(np.float32)
    Wq = np.random.randn(512, 1024).astype(np.float32) * 0.02
    K_ext = np.random.randn(8, 256, 16, 64).astype(np.float32)
    V_ext = np.random.randn(8, 256, 16, 64).astype(np.float32)
    Wo = np.random.randn(1024, 512).astype(np.float32) * 0.02
    return {"x": x, "Wq": Wq, "K_ext": K_ext, "V_ext": V_ext, "Wo": Wo}

def reference(x, Wq, K_ext, V_ext, Wo):
    B, Sq, Skv, Hq, Dh = 8, 256, 256, 16, 64
    Q = (x @ Wq).reshape(B, Sq, Hq, Dh)
    qb = (np.arange(Sq) // 64)[:, None]
    kb = (np.arange(Skv) // 64)[None, :]
    mask = (qb == kb) | ((kb % 4) == (qb % 4))
    scores = np.einsum('bihd,bjhd->bhij', Q, K_ext).astype(np.float32) * 0.125
    scores = np.where(mask[None, None, :, :], scores, -1e9)
    scores_max = scores.max(axis=-1, keepdims=True)
    w = np.exp(scores - scores_max)
    row_keep = mask.any(axis=1)
    w_sum = np.where(row_keep[None, None, :, None], w.sum(axis=-1, keepdims=True), 1.0)
    w = w / w_sum
    w = np.where(row_keep[None, None, :, None], w, 0.0)
    ctx = np.einsum('bhij,bjhd->bihd', w, V_ext).reshape(B, Sq, Hq * Dh)
    return ctx @ Wo
```

```python
import contextlib

import jax
import jax.numpy as jnp
from jax import lax
from jax.experimental import pallas as pl
from jax.experimental.pallas import tpu as pltpu

MESH = pl.DeviceIdType.MESH
BF = jnp.bfloat16
F32 = jnp.float32
LOG2E = 1.4426950408889634
OWN, LEFT, RIGHT, DIAG = 0, 1, 2, 3
NT = (((1,), (1,)), ((), ()))


def make(scopes=False, masked_q=True, out_dtype=BF):
    def scope(name):
        return jax.named_scope(name) if scopes else contextlib.nullcontext()

    def body(x_hbm, wq_hbm, kt_hbm, vt_hbm, wo_hbm, o_ref,
             xf, wqf, wof, ktf, vtf, xb, wq, wo, kb, vb, ctx, acc,
             lsem, ssem, rsem, ready):
        me = lax.axis_index("i")
        left = (me + 3) % 4
        right = (me + 1) % 4
        odd = (me % 2) == 1
        bar = pltpu.get_barrier_semaphore()

        FIRST = 64
        ld_q0 = pltpu.make_async_copy(wq_hbm.at[pl.ds(0, FIRST)], wqf.at[pl.ds(0, FIRST)], lsem.at[0])
        ld_q1 = pltpu.make_async_copy(wq_hbm.at[pl.ds(FIRST, 512 - FIRST)], wqf.at[pl.ds(FIRST, 512 - FIRST)], lsem.at[1])
        ld_o = pltpu.make_async_copy(wo_hbm, wof, lsem.at[2])
        ld_x = pltpu.make_async_copy(x_hbm, xf, lsem.at[3])
        ld_q0.start()

        @pl.when(me != 2)
        def _():
            pl.semaphore_signal(bar, 1, device_id=(left,), device_id_type=MESH)
            pl.semaphore_signal(bar, 1, device_id=(right,), device_id_type=MESH)

        ld_q1.start()
        ld_o.start()
        ld_x.start()
        ld_k, ld_v = [], []
        for s, src in enumerate((me, left, right, (me + 2) % 4)):
            rows = pl.ds(pl.multiple_of(src * 256, 256), 256)
            ld_k.append(pltpu.make_async_copy(kt_hbm.at[pl.ds(2 * me, 2), rows], ktf.at[s], lsem.at[4 + 2 * s]))
            ld_v.append(pltpu.make_async_copy(vt_hbm.at[pl.ds(2 * me, 2), rows], vtf.at[s], lsem.at[5 + 2 * s]))
            ld_k[s].start()
            ld_v[s].start()

        sent = []
        nsem = [0]

        def rcopy(src, dst, to_right):
            k = nsem[0]
            nsem[0] += 1
            cp = pltpu.make_async_remote_copy(src, dst, ssem.at[k], rsem.at[k],
                                              device_id=(right if to_right else left,), device_id_type=MESH)
            sent.append(cp)
            return cp

        r0, r1 = pl.ds(0, FIRST), pl.ds(FIRST, 512 - FIRST)
        q_r = [rcopy(wq.at[OWN, 0, r0], wq.at[LEFT, 0, r0], True), rcopy(wq.at[OWN, 0, r1], wq.at[LEFT, 0, r1], True),
               rcopy(wq.at[OWN, 1], wq.at[LEFT, 1], True)]
        q_l = [rcopy(wq.at[OWN, 1, r0], wq.at[RIGHT, 1, r0], False), rcopy(wq.at[OWN, 1, r1], wq.at[RIGHT, 1, r1], False),
               rcopy(wq.at[OWN, 0], wq.at[RIGHT, 0], False)]
        o_r = [rcopy(wo.at[OWN, 0], wo.at[LEFT, 0], True), rcopy(wo.at[OWN, 1], wo.at[LEFT, 1], True)]
        o_l = [rcopy(wo.at[OWN, 1], wo.at[RIGHT, 1], False), rcopy(wo.at[OWN, 0], wo.at[RIGHT, 0], False)]
        fq_r = rcopy(wq.at[LEFT, 0], wq.at[DIAG, 0], True)
        fq_l = rcopy(wq.at[RIGHT, 1], wq.at[DIAG, 1], False)
        fo_r = [rcopy(wo.at[LEFT, 0, n], wo.at[DIAG, 0, n], True) for n in range(4)]
        fo_l = [rcopy(wo.at[RIGHT, 1, n], wo.at[DIAG, 1, n], False) for n in range(4)]

        def cvt_q(rows):
            for u in range(2):
                wq[OWN, u, rows, :] = (wqf[rows, u * 128:(u + 1) * 128] * (0.125 * LOG2E)).astype(BF)

        with scope("ld_q0"):
            ld_q0.wait()
        cvt_q(r0)

        with scope("bar"):
            @pl.when(odd)
            def _():
                pl.semaphore_wait(bar, 1)

            @pl.when(jnp.logical_not(odd))
            def _():
                pl.semaphore_wait(bar, 2)

            @pl.when(me == 2)
            def _():
                pl.semaphore_signal(ready, 1, device_id=(left,), device_id_type=MESH)
                pl.semaphore_signal(ready, 1, device_id=(right,), device_id_type=MESH)

        @pl.when(me != 1)
        def _():
            q_r[0].start()

        @pl.when(me != 3)
        def _():
            q_l[0].start()

        with scope("ld_q1"):
            ld_q1.wait()
        cvt_q(r1)

        @pl.when(me != 1)
        def _():
            q_r[1].start()
            q_r[2].start()

        @pl.when(me != 3)
        def _():
            q_l[1].start()
            q_l[2].start()

        with scope("ready"):
            @pl.when(odd)
            def _():
                pl.semaphore_wait(ready, 1)

        @pl.when(me == 1)
        def _():
            for c in q_r:
                c.start()

        @pl.when(me == 3)
        def _():
            for c in q_l:
                c.start()

        with scope("ld_o"):
            ld_o.wait()
        for u in range(2):
            for n in range(4):
                wo[OWN, u, n] = wof[u * 128:(u + 1) * 128, n * 128:(n + 1) * 128].astype(BF)
        o_r[0].start()
        o_l[0].start()

        with scope("ld_x"):
            ld_x.wait()
        with scope("cvt_x"):
            for b in range(2):
                xb[b * 256:(b + 1) * 256, :] = xf[b].astype(BF)

        lane = lax.broadcasted_iota(jnp.int32, (64, 128), 1)
        lo = lane < 64

        def prep_kv(s):
            ld_k[s].wait()
            ld_v[s].wait()
            for b in range(2):
                for u in range(2):
                    for j in range(2):
                        kt = ktf[s, b, u * 128:(u + 1) * 128, j * 128:(j + 1) * 128]
                        k = kt.T
                        if masked_q:
                            kb[s, b, u, j, 0:64] = jnp.where(lo, k[:64], k[64:]).astype(BF)
                            kb[s, b, u, j, 64:128] = jnp.where(lo, k[64:], k[:64]).astype(BF)
                        else:
                            kb[s, b, u, j, 0:64] = jnp.where(lo, k[:64], 0.0).astype(BF)
                            kb[s, b, u, j, 64:128] = jnp.where(lo, k[64:], 0.0).astype(BF)
                            kb[s, b, u, j, 128:192] = jnp.where(lo, 0.0, k[:64]).astype(BF)
                            kb[s, b, u, j, 192:256] = jnp.where(lo, 0.0, k[64:]).astype(BF)
                vb[s, b] = vtf[s, b].astype(BF)

        def softmax_t(st):
            m = jnp.max(st, axis=0, keepdims=True)
            p = jnp.exp2(st - m)
            return p, jnp.sum(p, axis=0, keepdims=True)

        def attend(s, u):
            q = jnp.dot(xb[...], wq[s, u], preferred_element_type=F32)
            for b in range(2):
                for j in range(2):
                    r = b * 256 + j * 128
                    q0, q1 = q[r:r + 64], q[r + 64:r + 128]
                    if masked_q:
                        w1 = jnp.concatenate([jnp.where(lo, q0, 0.0), jnp.where(lo, 0.0, q1)], 0).astype(BF)
                        w2 = jnp.concatenate([jnp.where(lo, 0.0, q0), jnp.where(lo, q1, 0.0)], 0).astype(BF)
                        s1 = lax.dot_general(kb[s, b, u, j, 0:64], w1, NT, preferred_element_type=F32)
                        s2 = lax.dot_general(kb[s, b, u, j, 64:128], w2, NT, preferred_element_type=F32)
                        p1, l1 = softmax_t(s1)
                        p2, l2 = softmax_t(s2)
                        pw0 = jnp.concatenate([jnp.where(lo, p1, 0.0), jnp.where(lo, 0.0, p2)], 0).astype(BF)
                        pw1 = jnp.concatenate([jnp.where(lo, p2, 0.0), jnp.where(lo, 0.0, p1)], 0).astype(BF)
                        la = jnp.where(lo[:1], l1, l2)
                        lb = jnp.where(lo[:1], l2, l1)
                    else:
                        sa = lax.dot_general(kb[s, b, u, j], q[r:r + 128].astype(BF), NT, preferred_element_type=F32)
                        p1, la = softmax_t(jnp.where(lo, sa[0:64], sa[64:128]))
                        p2, lb = softmax_t(jnp.where(lo, sa[128:192], sa[192:256]))
                        pw0 = jnp.concatenate([jnp.where(lo, p1, 0.0), jnp.where(lo, 0.0, p1)], 0).astype(BF)
                        pw1 = jnp.concatenate([jnp.where(lo, p2, 0.0), jnp.where(lo, 0.0, p2)], 0).astype(BF)
                    v0 = vb[s, b, u * 128:u * 128 + 64, j * 128:(j + 1) * 128]
                    v1 = vb[s, b, u * 128 + 64:(u + 1) * 128, j * 128:(j + 1) * 128]
                    c0 = jnp.dot(v0, pw0, preferred_element_type=F32) * (1.0 / la)
                    c1 = jnp.dot(v1, pw1, preferred_element_type=F32) * (1.0 / lb)
                    ctx[s, u, r:r + 128, :] = jnp.concatenate([c0, c1], 0).T.astype(BF)

        def project(units, cols, first=False, last=False):
            lhs = jnp.concatenate([ctx[s, u] for s, u in units], axis=1)
            for n in cols:
                rhs = jnp.concatenate([wo[s, u, n] for s, u in units], axis=0)
                y = jnp.dot(lhs, rhs, preferred_element_type=F32)
                c = slice(n * 128, (n + 1) * 128)
                if not first:
                    y = y + acc[:, c]
                if last:
                    for b in range(2):
                        o_ref[b, :, c] = y[b * 256:(b + 1) * 256].astype(o_ref.dtype)
                else:
                    acc[:, c] = y

        with scope("prep0"):
            prep_kv(OWN)
        with scope("att_own"):
            attend(OWN, 0)
            attend(OWN, 1)
        with scope("w_q1"):
            for c in (q_r[0], q_r[1], q_l[0], q_l[1]):
                c.wait_recv()
        fq_r.start()
        fq_l.start()
        o_r[1].start()
        o_l[1].start()
        with scope("prep12"):
            prep_kv(LEFT)
            prep_kv(RIGHT)
        with scope("att_1"):
            attend(LEFT, 0)
            attend(RIGHT, 1)
        with scope("proj_own"):
            project([(OWN, 0), (OWN, 1)], range(4), first=True)
        with scope("w_q2"):
            q_r[2].wait_recv()
            q_l[2].wait_recv()
        with scope("att_2"):
            attend(LEFT, 1)
            attend(RIGHT, 0)
        with scope("prep3"):
            prep_kv(DIAG)
        with scope("w_o1"):
            o_r[0].wait_recv()
            o_l[0].wait_recv()
        for n in range(4):
            fo_r[n].start()
            fo_l[n].start()
        with scope("proj_1"):
            project([(LEFT, 0), (RIGHT, 1)], range(4))
        with scope("w_q3"):
            fq_r.wait_recv()
            fq_l.wait_recv()
        with scope("att_3"):
            attend(DIAG, 0)
            attend(DIAG, 1)
        with scope("w_o2"):
            o_r[1].wait_recv()
            o_l[1].wait_recv()
        with scope("proj_2"):
            project([(LEFT, 1), (RIGHT, 0)], range(4))
        for n in range(4):
            with scope(f"w_o3{n}"):
                fo_r[n].wait_recv()
                fo_l[n].wait_recv()
            if n == 3:
                for c in sent:
                    c.wait_send()
            with scope(f"proj_3{n}"):
                project([(DIAG, 0), (DIAG, 1)], [n], last=True)

    def fn(x, Wq, K_ext, V_ext, Wo):
        kt = jnp.transpose(K_ext, (0, 2, 3, 1)).reshape(8, 1024, 256)
        vt = jnp.transpose(V_ext, (0, 2, 3, 1)).reshape(8, 1024, 256)
        hbm = pl.BlockSpec(memory_space=pltpu.HBM)
        return pl.pallas_call(
            body,
            out_shape=jax.ShapeDtypeStruct(x.shape, out_dtype),
            in_specs=[hbm] * 5,
            out_specs=pl.BlockSpec(memory_space=pltpu.VMEM),
            scratch_shapes=[
                pltpu.VMEM((2, 256, 512), F32), pltpu.VMEM((512, 256), F32), pltpu.VMEM((256, 512), F32),
                pltpu.VMEM((4, 2, 256, 256), F32), pltpu.VMEM((4, 2, 256, 256), F32),
                pltpu.VMEM((512, 512), BF), pltpu.VMEM((4, 2, 512, 128), BF), pltpu.VMEM((4, 2, 4, 128, 128), BF),
                pltpu.VMEM((4, 2, 2, 2, 128 if masked_q else 256, 128), BF), pltpu.VMEM((4, 2, 256, 256), BF),
                pltpu.VMEM((4, 2, 512, 128), BF), pltpu.VMEM((512, 512), F32),
                pltpu.SemaphoreType.DMA((12,)), pltpu.SemaphoreType.DMA((20,)), pltpu.SemaphoreType.DMA((20,)),
                pltpu.SemaphoreType.REGULAR,
            ],
            compiler_params=pltpu.CompilerParams(
                collective_id=0, disable_bounds_checks=True, disable_semaphore_checks=True,
                vmem_limit_bytes=48 * 1024 * 1024),
        )(x, Wq, kt, vt, Wo)

    return fn


def pallas_dist_sparse_attn_strided_htp_bs_b2_sq256_skv256_hq4_dh64_kernel(x, Wq, K_ext, V_ext, Wo):
    return make()(x, Wq, K_ext, V_ext, Wo)
```

```python
import contextlib
import math

import jax
import jax.numpy as jnp
import numpy as np
from jax import lax
from jax.experimental import pallas as pl
from jax.experimental.pallas import tpu as pltpu

MESH = pl.DeviceIdType.MESH
BF = jnp.bfloat16
F32 = jnp.float32
I32 = jnp.int32
QSCALE = 0.125 * 1.4426950408889634
OWN, LEFT, RIGHT, DIAG = 0, 1, 2, 3
WQ, WO = 0, 1
NT = (((1,), (1,)), ((), ()))
NQ = 32
TOP = 10.8
HEADER = 112
SIGNS = (0, 160)


def i32(v):
    return np.uint32(v).astype(np.int32)


def rep(byte):
    return i32(byte * 0x01010101)


EVEN, ODD, MSB = i32(0x00FF00FF), i32(0xFF00FF00), i32(0x80000000)


def shl(v, n):
    return lax.shift_left(v, jnp.full_like(v, n) if isinstance(n, int) else n)


def shr(v, n):
    return lax.shift_right_logical(v, jnp.full_like(v, n) if isinstance(n, int) else n)


def words(v):
    return pltpu.bitcast(v.astype(BF), I32)


def halves(w):
    return pltpu.bitcast(w, BF)


def tile(j, n=1):
    return pl.ds(8 * j, 8 * n)


def window(t):
    mean, dev = 6.7 * t, 1.9 * math.sqrt(t)
    return max(math.floor((mean - dev) / 32), 0), math.floor((mean + 5.3 * dev + (10 if t else 0)) / 32) + 1


def word_row(i):
    return 32 + 8 * i if i < 10 else 40 + 8 * i


def mirrored(v):
    v = pltpu.roll(v, 4, 0)
    for k, mask in ((1, 0x55555555), (2, 0x33333333), (4, 0x0F0F0F0F), (8, 0x00FF00FF)):
        v = (shr(v, k) & mask) | shl(v & mask, k)
    return shr(v, 16) | shl(v, 16)


def make(scopes=False, out_dtype=BF, cuts=(2, 3, 5, 9), force_raw=False, half=False, tail=0, other=6, mid=160):
    assert window(NQ - 1)[1] <= 9 and window(NQ)[0] >= 6
    npair = 31 if half else 30

    def scope(name):
        return jax.named_scope(name) if scopes else contextlib.nullcontext()

    def body(x_hbm, wq_hbm, kt_hbm, vt_hbm, wo_hbm, o_ref,
             xf, wqf, wof, ktf, vtf, xb, lo_b, code, hi_b, hi_raw, stage, kb, vb, ctx, acc,
             lsem, ssem, rsem, ready):
        me = lax.axis_index("i")
        left = (me + 3) & 3
        right = (me + 1) & 3
        odd = (me & 1) == 1
        bar = pltpu.get_barrier_semaphore()

        nsem = [0]

        def rcopy(src, dst, to_right):
            k = nsem[0]
            nsem[0] += 1
            return pltpu.make_async_remote_copy(src, dst, ssem.at[k], rsem.at[k],
                                                device_id=(right if to_right else left,), device_id_type=MESH)

        def both(buf, rows_r, rows_l):
            return (rcopy(buf.at[OWN, rows_r], buf.at[LEFT, rows_r], True),
                    rcopy(buf.at[OWN, rows_l], buf.at[RIGHT, rows_l], False))

        def onward(buf, rows_r, rows_l):
            return (rcopy(buf.at[LEFT, rows_r], buf.at[DIAG, rows_r], True),
                    rcopy(buf.at[RIGHT, rows_l], buf.at[DIAG, rows_l], False))

        def first_half(u, a, n, k):
            rows = pl.ds(pl.multiple_of(128 * u + 8 * a, 8), 8 * n)
            return pltpu.make_async_remote_copy(
                lo_b.at[OWN, rows], lo_b.at[LEFT + u, rows], ssem.at[k + u], rsem.at[k + u],
                device_id=((me + 1 + 2 * u) & 3,), device_id_type=MESH)

        def unrounded(u):
            return pltpu.make_async_remote_copy(
                wq_hbm.at[pl.ds(0, 32), pl.ds(pl.multiple_of(128 * u, 128), 128)], stage.at[u], ssem.at[4], rsem.at[4 + u],
                device_id=(0,), device_id_type=MESH)

        nsem[0] = 6
        end = 196 if half else 192
        c_h1 = both(code, pl.ds(0, 80), pl.ds(0, 80))
        c_h2 = both(code, pl.ds(80, 33), pl.ds(80, 33))
        c_q2 = both(lo_b, tile(16, 16), tile(0, 16))
        c_ho = both(code, pl.ds(120, end - 120), pl.ds(120, end - 120))
        c_o1 = [both(lo_b, tile(32 + a, n), tile(48 + a, n)) for a, n in ((0, 4), (4, 8), (12, 4))]
        f_hq = onward(code, pl.ds(0, 56), pl.ds(56, 57))
        f_q = onward(lo_b, tile(0, 16), tile(16, 16))
        f_ho = onward(code, pl.ds(120, mid - 120), pl.ds(mid, end - mid))
        c_o2 = [both(lo_b, tile(48 + 8 * n, 8), tile(32 + 8 * n, 8)) for n in range(2)]
        f_o = [onward(lo_b, tile(32 + 4 * n, 4), tile(48 + 4 * n, 4)) for n in range(3 if tail else 4)]
        if tail:
            f_o += [onward(lo_b, tile(44 + 2 * h, 2), tile(60 + 2 * h, 2)) for h in range(2)]
        raw = (rcopy(hi_b.at[OWN], hi_raw.at[LEFT], True), rcopy(hi_b.at[OWN], hi_raw.at[RIGHT], False),
               rcopy(hi_raw.at[LEFT], hi_raw.at[DIAG], True))

        def start(*pairs):
            for p in pairs:
                p[0].start()
                p[1].start()

        def arrived(*pairs):
            for p in pairs:
                p[0].wait_recv()
                p[1].wait_recv()

        def drained(*pairs):
            for p in pairs:
                p[0].wait_send()
                p[1].wait_send()

        lead = jnp.where(me == 1, 1, 0)
        spans = list(zip((1,) + cuts, cuts + (16,)))

        def load_q(slot, u, a, b, k):
            rows = pl.ds(32 * a, 32 * (b - a))
            return pltpu.make_async_copy(wq_hbm.at[rows, pl.ds(pl.multiple_of(128 * u, 128), 128)],
                                         wqf.at[slot, rows], lsem.at[k])

        ld_q = [load_q(0, lead, a, b, 20 + i) for i, (a, b) in enumerate(spans)]
        ld_q0 = load_q(0, lead, 0, 1, 0)
        ld_q1 = load_q(1, 1 - lead, 0, other, 19)
        ld_q2 = load_q(1, 1 - lead, other, 16, 1)
        ld_o = pltpu.make_async_copy(wo_hbm, wof, lsem.at[2])
        ld_x = pltpu.make_async_copy(x_hbm, xf, lsem.at[3])
        ld_q[0].start()

        @pl.when(odd)
        def _():
            pl.semaphore_wait(bar, 1)
            unrounded(lead).start()

        @pl.when(me != 2)
        def _():
            pl.semaphore_signal(bar, 1, device_id=(left,), device_id_type=MESH)
            pl.semaphore_signal(bar, 1, device_id=(right,), device_id_type=MESH)

        for c in ld_q[1:-1] + [ld_q1, ld_q[-1], ld_q0, ld_q2, ld_o, ld_x]:
            c.start()
        owner = (me, left, right, (me + 2) & 3)
        ld_kv = {}
        for s, u in ((OWN, 0), (OWN, 1), (LEFT, 0), (RIGHT, 1), (LEFT, 1), (RIGHT, 0), (DIAG, 0), (DIAG, 1)):
            rows = pl.ds(pl.multiple_of(owner[s] * 256 + u * 128, 128), 128)
            k = 28 + 4 * s + 2 * u
            ld_kv[s, u] = (
                pltpu.make_async_copy(kt_hbm.at[pl.ds(2 * me, 2), rows], ktf.at[s, u], lsem.at[k]),
                pltpu.make_async_copy(vt_hbm.at[pl.ds(2 * me, 2), rows], vtf.at[s, u], lsem.at[k + 1]))
            for c in ld_kv[s, u]:
                c.start()

        with scope("bar"):
            @pl.when(jnp.logical_not(odd))
            def _():
                pl.semaphore_wait(bar, 2)

                @pl.when(me == 2)
                def _():
                    pl.semaphore_signal(ready, 1, device_id=(left,), device_id_type=MESH)
                    pl.semaphore_signal(ready, 1, device_id=(right,), device_id_type=MESH)

        def planes(v):
            w = words(v)
            a, b = w[:8], w[8:]
            return (a & EVEN) | (shl(b, 8) & ODD), (shr(a, 8) & EVEN) | (b & ODD)

        def split(v, t):
            rows = pl.ds(t * 8 if isinstance(t, int) else pl.multiple_of(t * 8, 8), 8)
            lo_b[OWN, rows], hi_b[OWN, rows] = planes(v)
            return jnp.abs(v)

        def split_q(slot, u, tiles_):
            return sum(split(wqf[slot, 32 * i:32 * i + 32] * QSCALE, 16 * u + i) for i in tiles_)

        def pivot_of(total):
            top = jnp.sum(total, axis=0, keepdims=True) * (TOP / (32 * NQ))
            return shr(pltpu.bitcast(jnp.broadcast_to(top, (8, 128)), I32), 16) | 0x8000

        def expand(pivot):
            def spread(v):
                v = v | shl(v, 8)
                return v | shl(v, 16)
            return spread(shr(pivot, 8)), spread(127 - shr(pivot & 0xFF, 1))

        def flip(h, l, ref):
            return ref[0] - h - (shr((shr(l, 1) & rep(0x7F)) + ref[1], 7) & rep(0x01))

        zero = jnp.zeros((8, 128), I32)

        def encode(m, pivot, state):
            pos, bad, out = state
            ref = expand(pivot)
            for t in range(NQ * m, NQ * m + NQ):
                h = flip(hi_b[OWN, tile(t)], lo_b[OWN, tile(t)], ref)
                hi_b[OWN, tile(t)] = h
                sg = h & rep(0x80)
                signs = sg if t % 8 == 0 else signs | shr(sg, t % 8)
                if t % 8 == 7:
                    code[OWN, pl.ds(SIGNS[m] + t % NQ - 7, 8)] = signs
                d = h & rep(0x7F)
                n = d + (shr(d + rep(0x7C), 7) & rep(0x01)) + (shr(rep(0x80) - d, 5) & rep(0x04))
                n0, n1, n2, n3 = n & 31, shr(n, 8) & 31, shr(n, 16) & 31, shr(n, 24) & 31
                win = shr(shr(shr(shr(zero + MSB, n3) | MSB, n2) | MSB, n1) | MSB, (n0 - 1) & 31)
                length = (n0 + n1) + (n2 + n3)
                lo, hi = window(t)
                if t and lo > window(t - 1)[0]:
                    pos = jnp.maximum(pos, 32 * lo)
                    if lo - 1 < 12:
                        code[OWN, pl.ds(word_row(lo - 1), 8)] = out.pop(lo - 1)
                bad = bad | (n & rep(0xE0)) | ((32 - length) & MSB)
                if window(t + 1)[1] > hi or t == 2 * NQ - 1:
                    bad = bad | ((32 * hi - 1 - pos) & MSB)
                sh, k = pos & 31, shr(pos, 5)
                head, rest = shr(win, sh), shl(shl(win, 1), 31 - sh)
                for i in range(lo, hi + 1):
                    v = jnp.where(k == i - 1, rest, 0) if i > lo else zero
                    v = jnp.where(k == i, head, v) if i < hi else v
                    out[i] = out[i] | v if i in out else v
                pos = pos + length
            return pos, bad, out

        def finish(state, piv_q, piv_o):
            pos, bad, out = state
            for i in sorted(out):
                if 2 * i < npair:
                    j = npair - 1 - i
                    v = out[i] | mirrored(out[j]) if j in out else out[i]
                    if i == j:
                        code[OWN, pl.ds(192, 4)] = v[:4]
                    else:
                        code[OWN, pl.ds(word_row(i), 8)] = v
            bad = bad | ((32 * npair - pos - pltpu.roll(pos, 4, 0)) & MSB)
            bad = jnp.where(bad != 0, 1.0, 0.0)
            bad = jnp.max(jnp.max(bad, axis=0, keepdims=True), axis=1, keepdims=True)
            if force_raw:
                bad = bad + 1.0
            both_p = (piv_q | shl(piv_o, 16))[:1]
            code[OWN, pl.ds(HEADER, 1)] = jnp.where(bad > 0.0, both_p & 0x7FFFFFFF, both_p)

        def overflowed(s):
            return code[s, pl.ds(HEADER, 1)][0, 0] >= 0

        def pivot_from(s, m):
            k = jnp.broadcast_to(code[s, pl.ds(HEADER, 1)], (8, 128))
            return expand((k & 0xFFFF) if m == WQ else (shr(k, 16) | 0x8000))

        def decode(m, state):
            cache = {}

            def word(s, i):
                if (s, i) not in cache:
                    if 2 * i + 1 < npair:
                        cache[s, i] = code[s, pl.ds(word_row(i), 8)]
                    elif 2 * i + 1 == npair:
                        v = code[s, pl.ds(192, 4)]
                        v = jnp.concatenate([v, v], axis=0)
                        cache[s, i] = jnp.where(lax.broadcasted_iota(I32, v.shape, 0) < 4, v, mirrored(v))
                    else:
                        cache[s, i] = mirrored(word(s, npair - 1 - i))
                return cache[s, i]

            state = dict(state)
            for t in range(NQ * m, NQ * m + NQ):
                lo, hi = window(t)
                for s, pos in state.items():
                    if t and lo > window(t - 1)[0]:
                        pos = jnp.maximum(pos, 32 * lo)
                    a, b = word(s, lo), word(s, lo + 1)
                    for i in range(lo + 1, hi):
                        past = pos >= 32 * i
                        a, b = jnp.where(past, word(s, i), a), jnp.where(past, word(s, i + 1), b)
                    sh = pos & 31
                    win = shl(a, sh) | shr(shr(b, 1), 31 - sh)
                    z0 = lax.clz(win)
                    win = shl(shl(win, 1), z0)
                    z1 = lax.clz(win)
                    win = shl(shl(win, 1), z1)
                    z2 = lax.clz(win)
                    z3 = lax.clz(shl(shl(win, 1), z2))
                    state[s] = (pos + 4 + z0) + (z1 + z2) + z3
                    z = (z0 | shl(z1, 8)) | (shl(z2, 16) | shl(z3, 24))
                    lt4 = shr(rep(0x83) - z, 7) & rep(0x01)
                    d = (z + lt4) & ~shl(lt4, 2)
                    sg = code[s, pl.ds(SIGNS[m] + t % NQ // 8 * 8, 8)]
                    hi_b[s, tile(t)] = d | ((shl(sg, t % 8) if t % 8 else sg) & rep(0x80))
            return state

        def take_raw(s, m, flag):
            @pl.when(flag)
            def _():
                if m == WQ:
                    raw[s - 1].wait_recv()
                    if s == LEFT:
                        raw[2].start()
                hi_b[s, tile(NQ * m, NQ)] = hi_raw[s, tile(NQ * m, NQ)]

        def weights(s, quads, ref=None):
            ref = ref or pivot_from(s, quads[0] // NQ)
            out = []
            for t in quads:
                l = lo_b[s, tile(t)]
                h = flip(hi_b[s, tile(t)], l, ref)
                out.append((l & EVEN) | (shl(h, 8) & ODD))
                out.append((shr(l, 8) & EVEN) | (h & ODD))
            return halves(jnp.concatenate(out, axis=0))

        lo = lax.broadcasted_iota(I32, (64, 128), 1) < 64
        tiles = [(b, j) for b in range(2) for j in range(2)]

        def prep_kv(s, u):
            for b, j in tiles:
                k = ktf[s, u, b, :, 128 * j:128 * j + 128].T
                kb[s, u, b, j, 0:32] = words(jnp.where(lo, k[:64], k[64:]))
                kb[s, u, b, j, 32:64] = words(jnp.where(lo, k[64:], k[:64]))
                vb[s, u, b, j] = words(vtf[s, u, b, :, 128 * j:128 * j + 128])

        def wait_kv(*units):
            for su in units:
                for c in ld_kv[su]:
                    c.wait()

        def q_proj(s, u):
            return jnp.dot(halves(xb[...]), weights(s, range(16 * u, 16 * u + 16)), preferred_element_type=F32)

        def diag2(a, b):
            return jnp.concatenate([jnp.where(lo, a, 0.0), jnp.where(lo, 0.0, b)], 0).astype(BF)

        def scores(s, u, q):
            out = []
            for b, j in tiles:
                r = 256 * b + 128 * j
                q0, q1 = q[r:r + 64], q[r + 64:r + 128]
                anti = jnp.concatenate([jnp.where(lo, 0.0, q0), jnp.where(lo, q1, 0.0)], 0).astype(BF)
                out.append((lax.dot_general(halves(kb[s, u, b, j, 0:32]), diag2(q0, q1), NT, preferred_element_type=F32),
                            lax.dot_general(halves(kb[s, u, b, j, 32:64]), anti, NT, preferred_element_type=F32)))
            return out

        def softmax_t(st):
            p = jnp.exp2(st - jnp.max(st, axis=0, keepdims=True))
            return p, 1.0 / jnp.sum(p, axis=0, keepdims=True)

        def values(s, u, sc):
            for (b, j), (s1, s2) in zip(tiles, sc):
                p1, i1 = softmax_t(s1)
                p2, i2 = softmax_t(s2)
                c0 = jnp.dot(halves(vb[s, u, b, j, 0:32]), diag2(p1, p2), preferred_element_type=F32)
                c1 = jnp.dot(halves(vb[s, u, b, j, 32:64]), diag2(p2, p1), preferred_element_type=F32)
                c = jnp.concatenate([c0 * jnp.where(lo[:1], i1, i2), c1 * jnp.where(lo[:1], i2, i1)], 0)
                ctx[s, u, pl.ds(128 * b + 64 * j, 64)] = words(c.T)

        def partial(units, n, ref=None):
            lhs = jnp.concatenate([halves(ctx[s, u]) for s, u in units], axis=1)
            rhs = jnp.concatenate([weights(s, range(32 + 16 * u + 4 * n, 36 + 16 * u + 4 * n), ref) for s, u in units], axis=0)
            return jnp.concatenate([jnp.dot(lhs[r:r + 256], rhs, preferred_element_type=F32) for r in (0, 256)], axis=0)

        def project(units, n, first=False):
            c = slice(128 * n, 128 * n + 128)
            y = partial(units, n)
            acc[:, c] = y if first else y + acc[:, c]

        def emit(y, n):
            c = slice(128 * n, 128 * n + 128)
            for b in range(2):
                o_ref[b, :, c] = (y[256 * b:256 * b + 256] + acc[256 * b:256 * b + 256, c]).astype(o_ref.dtype)

        def step(unit, prev=None, prep=True):
            if prep:
                prep_kv(*unit)
            q = q_proj(*unit)
            if prev is not None:
                values(*prev)
            return (*unit, scores(*unit, q))

        total = 0.0
        even = jnp.logical_not(odd)
        for i, (a, b) in enumerate(spans):
            if b == 16:
                ld_q1.wait()
                total = total + split_q(1, 1 - lead, range(other))

                @pl.when(even)
                def _():
                    first_half(1 - lead, 0, 1, 2).start()
                    first_half(1 - lead, 1, other - 1, 0).start()

            with scope(f"ld_q{i}"):
                ld_q[i].wait()
            total = total + split_q(0, lead, range(a, b))
            first_half(lead, a, b - a, 0).start()
        ld_q0.wait()
        total = total + split_q(0, lead, [0])
        pl.when(even)(lambda: first_half(lead, 0, 1, 2).start())
        with scope("ld_qb"):
            ld_q2.wait()
        total = total + split_q(1, 1 - lead, range(other, 16))
        pl.when(even)(lambda: first_half(1 - lead, other, 16 - other, 0).start())
        with scope("enc_q"):
            piv_q = pivot_of(total)
            state = encode(WQ, piv_q, (zero, zero, {}))
        with scope("ready"):
            @pl.when(odd)
            def _():
                pl.semaphore_wait(ready, 1)
                first_half(1 - lead, 0, 1, 2).start()
                first_half(1 - lead, 1, 15, 0).start()

        start(c_h1)
        with scope("ld_o"):
            ld_o.wait()
        with scope("enc_o"):
            piv_o = pivot_of(sum(
                split(wof[128 * u + 32 * i:128 * u + 32 * i + 32, 128 * n:128 * n + 128], NQ + 16 * u + 4 * n + i)
                for u in range(2) for n in range(4) for i in range(4)))
            finish(encode(WO, piv_o, state), piv_q, piv_o)
        start(c_h2, c_ho, c_q2, c_o1[0])
        bad = {OWN: overflowed(OWN)}
        pl.when(bad[OWN])(lambda: start(raw))

        with scope("ld_x"):
            ld_x.wait()
        with scope("q_own"):
            for b in range(2):
                xb[128 * b:128 * b + 128] = words(xf[b])
            qa = q_proj(OWN, 0)
            qb = q_proj(OWN, 1)
        with scope("ld_kv0"):
            wait_kv((OWN, 0))
        with scope("B1"):
            prep_kv(OWN, 0)
            sa = scores(OWN, 0, qa)
        with scope("ld_kv0b"):
            wait_kv((OWN, 1))
        with scope("B2"):
            prep_kv(OWN, 1)
            values(OWN, 0, sa)
            values(OWN, 1, scores(OWN, 1, qb))
        @pl.when(me == 0)
        def _():
            for u in range(2):
                unrounded(u).wait_recv()
                lo_b[LEFT + u, tile(16 * u)] = planes(stage[u] * QSCALE)[0]

        @pl.when(me != 0)
        def _():
            for u in range(2):
                first_half(u, 0, 1, 2).wait_recv()

        with scope("w_hq"):
            for u in range(2):
                first_half(u, 1, 15, 0).wait_recv()
            arrived(c_h1, c_h2)
        start(f_hq, f_q, *c_o1[1:])
        with scope("B3"):
            for s in (LEFT, RIGHT):
                bad[s] = overflowed(s)
            near = decode(WQ, {LEFT: zero, RIGHT: zero})
            for n in range(4):
                project([(OWN, 0), (OWN, 1)], n, first=True)
        take_raw(LEFT, WQ, bad[LEFT])
        take_raw(RIGHT, WQ, bad[RIGHT])
        with scope("ld_kv1"):
            arrived(c_ho)
            wait_kv((LEFT, 0), (RIGHT, 1))
        start(f_ho, *c_o2)
        with scope("B4"):
            decode(WO, {LEFT: near[LEFT]})
            pend = step((RIGHT, 1), step((LEFT, 0)))
        with scope("w_q2"):
            arrived(c_q2)
            wait_kv((LEFT, 1), (RIGHT, 0))
        with scope("B5"):
            decode(WO, {RIGHT: near[RIGHT]})
            pend = step((RIGHT, 0), step((LEFT, 1), pend))
        take_raw(LEFT, WO, bad[LEFT])
        take_raw(RIGHT, WO, bad[RIGHT])
        with scope("w_fhq"):
            arrived(f_hq, c_o1[0])
            wait_kv((DIAG, 0), (DIAG, 1))
        start(f_o[0])
        with scope("B7"):
            bad[DIAG] = overflowed(DIAG)
            far = decode(WQ, {DIAG: zero})
            values(*pend)
            prep_kv(DIAG, 0)
            prep_kv(DIAG, 1)
            project([(LEFT, 0), (RIGHT, 1)], 0)
        take_raw(DIAG, WQ, bad[DIAG])
        with scope("w_fq"):
            drained(c_h1, c_h2, c_q2, c_ho, c_o1[0])
            for u in range(2):
                first_half(u, 1, 15, 0).wait_send()
            first_half(1 - lead, 0, 1, 2).wait_send()
            pl.when(even)(lambda: first_half(lead, 0, 1, 2).wait_send())
            pl.when(odd)(lambda: unrounded(lead).wait_send())
            arrived(f_q)
        with scope("B8a"):
            pend = step((DIAG, 0), prep=False)
        with scope("w_o1"):
            arrived(c_o1[1])
        start(*f_o[1:3])
        with scope("B8b"):
            pend = step((DIAG, 1), pend, prep=False)
            project([(LEFT, 0), (RIGHT, 1)], 1)
        with scope("w_fho"):
            arrived(c_o1[2])
            start(*f_o[3:])
            arrived(f_ho)
        with scope("B9"):
            decode(WO, far)
            values(*pend)
            for n in range(2, 4):
                project([(LEFT, 0), (RIGHT, 1)], n)
        take_raw(DIAG, WO, bad[DIAG])
        with scope("w_o2a"):
            arrived(c_o2[0])
        with scope("B10"):
            for n in range(2):
                project([(LEFT, 1), (RIGHT, 0)], n)
            if tail:
                c0, c1 = ctx[DIAG, 0], ctx[DIAG, 1]
                low = lax.broadcasted_iota(I32, c0.shape, 1) < 64
                ctx[OWN, 0] = jnp.where(low, c0, pltpu.roll(c1, 64, 1))
                ctx[OWN, 1] = jnp.where(low, pltpu.roll(c0, 64, 1), c1)
        with scope("w_o2b"):
            drained(f_hq, f_q, *c_o1[1:], f_ho, c_o2[0])
            pl.when(bad[OWN])(lambda: drained(raw))
            pl.when(bad[LEFT])(raw[2].wait_send)
            arrived(c_o2[1])
        with scope("B11"):
            ref = pivot_from(DIAG, WO)
            for n in range(2, 4):
                project([(LEFT, 1), (RIGHT, 0)], n)
        last = [(DIAG, 0), (DIAG, 1)]
        for n in range(3):
            with scope(f"w_o3{n}"):
                arrived(f_o[n])
            y = partial(last, n, ref)
            if n < 2 or tail < 2:
                emit(y, n)
        if not tail:
            drained(c_o2[1], *f_o[:3])
            arrived(f_o[3])
            emit(partial(last, 3, ref), 3)
            drained(f_o[3])
        else:
            def part(h):
                rhs = weights(DIAG, [44 + 2 * h, 45 + 2 * h, 60 + 2 * h, 61 + 2 * h], ref)
                return jnp.concatenate([jnp.dot(halves(ctx[OWN, h, 64 * p:64 * p + 64]), rhs, preferred_element_type=F32)
                                        for p in range(4)], axis=0)

            arrived(f_o[3])
            y0 = part(0)
            if tail == 2:
                emit(y, 2)
            drained(c_o2[1], *f_o[:4])
            arrived(f_o[4])
            emit(y0 + part(1), 3)
            drained(f_o[4])

    def fn(x, Wq, K_ext, V_ext, Wo):
        kt = jnp.transpose(K_ext, (0, 2, 3, 1)).reshape(8, 1024, 256)
        vt = jnp.transpose(V_ext, (0, 2, 3, 1)).reshape(8, 1024, 256)
        hbm = pl.BlockSpec(memory_space=pltpu.HBM)
        plane = pltpu.VMEM((4, 16 * NQ, 128), I32)
        return pl.pallas_call(
            body,
            out_shape=jax.ShapeDtypeStruct(x.shape, out_dtype),
            in_specs=[hbm] * 5,
            out_specs=pl.BlockSpec(memory_space=pltpu.VMEM),
            scratch_shapes=[
                pltpu.VMEM((2, 256, 512), F32), pltpu.VMEM((2, 512, 128), F32), pltpu.VMEM((256, 512), F32),
                pltpu.VMEM((4, 2, 2, 128, 256), F32), pltpu.VMEM((4, 2, 2, 128, 256), F32),
                pltpu.VMEM((256, 512), I32), plane, pltpu.VMEM((4, 200, 128), I32), plane, plane,
                pltpu.VMEM((2, 32, 128), F32),
                pltpu.VMEM((4, 2, 2, 2, 64, 128), I32), pltpu.VMEM((4, 2, 2, 2, 64, 128), I32),
                pltpu.VMEM((4, 2, 256, 128), I32), pltpu.VMEM((512, 512), F32),
                pltpu.SemaphoreType.DMA((44,)), pltpu.SemaphoreType.DMA((52,)), pltpu.SemaphoreType.DMA((52,)),
                pltpu.SemaphoreType.REGULAR,
            ],
            compiler_params=pltpu.CompilerParams(
                collective_id=0, disable_bounds_checks=True, disable_semaphore_checks=True,
                vmem_limit_bytes=48 * 1024 * 1024),
        )(x, Wq, kt, vt, Wo)

    return fn


def pallas_dist_sparse_attn_strided_htp_bs_b2_sq256_skv256_hq4_dh64_kernel(x, Wq, K_ext, V_ext, Wo):
    return make()(x, Wq, K_ext, V_ext, Wo)
```

```python
import math

import jax
import jax.numpy as jnp
import numpy as np
from jax import lax
from jax.experimental import pallas as pl
from jax.experimental.pallas import tpu as pltpu

BF16, F32, I32 = jnp.bfloat16, jnp.float32, jnp.int32
MESH = pl.DeviceIdType.MESH
Q_SCALE = 0.125 * math.log2(math.e)
OWN, LEFT, RIGHT, FAR = 0, 1, 2, 3
WQ, WO = 0, 1

QUADS = 32
STREAM_WORDS = 15
PIVOT_RATIO = 10.8
SIGN_ROW, HEADER_ROW, CODE_ROWS = (0, 160), 112, 192


def _i32(v):
    return np.uint32(v).astype(np.int32)


def _bytes(b):
    return _i32(b * 0x01010101)


EVEN, ODD, TOP_BIT = _i32(0x00FF00FF), _i32(0xFF00FF00), _i32(0x80000000)


def _shl(v, n):
    return lax.shift_left(v, jnp.full_like(v, n) if isinstance(n, int) else n)


def _shr(v, n):
    return lax.shift_right_logical(v, jnp.full_like(v, n) if isinstance(n, int) else n)


def _words(v):
    return pltpu.bitcast(v.astype(BF16), I32)


def _halves(w):
    return pltpu.bitcast(w, BF16)


def _aligned(start, size, align):
    return pl.ds(start if isinstance(start, int) else pl.multiple_of(start, align), size)


def _quads(first, n=1):
    return _aligned(8 * first, 8 * n, 8)


def _stream_word(i):
    return pl.ds(32 + 8 * i if i < 10 else 40 + 8 * i, 8)


def _window(t):
    mean, dev = 6.7 * t, 1.9 * math.sqrt(t)
    return (max(math.floor((mean - dev) / 32), 0),
            math.floor((mean + 5.3 * dev + (10 if t else 0)) / 32) + 1)


def _mirrored(v):
    v = pltpu.roll(v, 4, 0)
    for k, mask in ((1, 0x55555555), (2, 0x33333333), (4, 0x0F0F0F0F), (8, 0x00FF00FF)):
        v = (_shr(v, k) & mask) | _shl(v & mask, k)
    return _shr(v, 16) | _shl(v, 16)


def _interleave(a, b):
    return (a & EVEN) | (_shl(b, 8) & ODD), (_shr(a, 8) & EVEN) | (b & ODD)


def _pivot_bytes(pivot):
    def spread(v):
        v = v | _shl(v, 8)
        return v | _shl(v, 16)
    return spread(_shr(pivot, 8)), spread(127 - _shr(pivot & 0xFF, 1))


def _from_pivot(high, low, pivot_bytes):
    borrow = _shr((_shr(low, 1) & _bytes(0x7F)) + pivot_bytes[1], 7) & _bytes(0x01)
    return pivot_bytes[0] - high - borrow


def _body(x_hbm, wq_hbm, kt_hbm, vt_hbm, wo_hbm, o_ref,
          x_f32, wq_f32, wo_f32, kt_f32, vt_f32, early, low, high, uncoded, code, xb, kb, vb, ctx, acc,
          load_sem, send_sem, recv_sem, ready):
    me = lax.axis_index("i")
    left, right = (me + 3) & 3, (me + 1) & 3
    odd = (me & 1) == 1
    even = jnp.logical_not(odd)
    barrier = pltpu.get_barrier_semaphore()

    def remote(src, dst, k, to):
        return pltpu.make_async_remote_copy(src, dst, send_sem.at[k], recv_sem.at[k],
                                            device_id=(to,), device_id_type=MESH)

    def first_pair(u, a, n, k):
        rows = _quads(16 * u + a, n)
        return remote(low.at[OWN, rows], low.at[LEFT + u, rows], k + u, (me + 1 + 2 * u) & 3)

    def unrounded(u):
        return remote(wq_hbm.at[pl.ds(0, 32), _aligned(128 * u, 128, 128)], early.at[u], 4 + u, 0)

    free_sems = iter(range(6, send_sem.shape[0]))

    def mine(buf, rows_r, rows_l, dst=None):
        dst = buf if dst is None else dst
        return (remote(buf.at[OWN, rows_r], dst.at[LEFT, rows_r], next(free_sems), right),
                remote(buf.at[OWN, rows_l], dst.at[RIGHT, rows_l], next(free_sems), left))

    def onward(buf, rows_r, rows_l):
        return (remote(buf.at[LEFT, rows_r], buf.at[FAR, rows_r], next(free_sems), right),
                remote(buf.at[RIGHT, rows_l], buf.at[FAR, rows_l], next(free_sems), left))

    code_q1 = mine(code, pl.ds(0, 80), pl.ds(0, 80))
    code_q2 = mine(code, pl.ds(80, 33), pl.ds(80, 33))
    code_o = mine(code, pl.ds(120, 72), pl.ds(120, 72))
    low_q2 = mine(low, _quads(16, 16), _quads(0, 16))
    low_o1 = [mine(low, _quads(32 + a, n), _quads(48 + a, n)) for a, n in ((0, 4), (4, 8), (12, 4))]
    low_o2 = [mine(low, _quads(48 + a, 8), _quads(32 + a, 8)) for a in (0, 8)]
    far_code_q = onward(code, pl.ds(0, 56), pl.ds(56, 57))
    far_code_o = onward(code, pl.ds(120, 40), pl.ds(160, 32))
    far_low_q = onward(low, _quads(0, 16), _quads(16, 16))
    far_low_o = [onward(low, _quads(32 + 4 * n, 4), _quads(48 + 4 * n, 4)) for n in range(4)]
    plain = [mine(high, _quads(QUADS * m, QUADS), _quads(QUADS * m, QUADS), uncoded) for m in (WQ, WO)]
    far_plain = [onward(uncoded, _quads(QUADS * m, 16), _quads(QUADS * m + 16, 16)) for m in (WQ, WO)]

    def start(*pairs):
        for pair in pairs:
            for copy in pair:
                copy.start()

    def arrived(*pairs):
        for pair in pairs:
            for copy in pair:
                copy.wait_recv()

    def drained(*pairs):
        for pair in pairs:
            for copy in pair:
                copy.wait_send()

    lead = jnp.where(me == 1, 1, 0)
    spans = ((1, 2), (2, 3), (3, 5), (5, 9), (9, 16))
    free_loads = iter(range(load_sem.shape[0]))

    def load(src, dst):
        return pltpu.make_async_copy(src, dst, load_sem.at[next(free_loads)])

    def load_wq(slot, u, a, b):
        rows = pl.ds(32 * a, 32 * (b - a))
        return load(wq_hbm.at[rows, _aligned(128 * u, 128, 128)], wq_f32.at[slot, rows])

    load_lead = [load_wq(0, lead, a, b) for a, b in spans]
    load_lead0 = load_wq(0, lead, 0, 1)
    load_other = [load_wq(1, 1 - lead, 0, 6), load_wq(1, 1 - lead, 6, 16)]
    load_wo, load_x = load(wo_hbm, wo_f32), load(x_hbm, x_f32)
    load_lead[0].start()

    @pl.when(odd)
    def _():
        pl.semaphore_wait(barrier, 1)
        unrounded(lead).start()

    @pl.when(me != 2)
    def _():
        for to in (left, right):
            pl.semaphore_signal(barrier, 1, device_id=(to,), device_id_type=MESH)

    for copy in (*load_lead[1:-1], load_other[0], load_lead[-1], load_lead0, load_other[1], load_wo, load_x):
        copy.start()
    owner = (me, left, right, (me + 2) & 3)
    load_kv = {}
    for s, u in ((OWN, 0), (OWN, 1), (LEFT, 0), (RIGHT, 1), (LEFT, 1), (RIGHT, 0), (FAR, 0), (FAR, 1)):
        part = (pl.ds(2 * me, 2), _aligned(256 * owner[s] + 128 * u, 128, 128))
        load_kv[s, u] = (load(kt_hbm.at[part], kt_f32.at[s, u]), load(vt_hbm.at[part], vt_f32.at[s, u]))
        start(load_kv[s, u])

    @pl.when(even)
    def _():
        pl.semaphore_wait(barrier, 2)

        @pl.when(me == 2)
        def _():
            for to in (left, right):
                pl.semaphore_signal(ready, 1, device_id=(to,), device_id_type=MESH)

    zero = jnp.zeros((8, 128), I32)

    def split(v, t):
        w = _words(v)
        low[OWN, _quads(t)], high[OWN, _quads(t)] = _interleave(w[:8], w[8:])
        return jnp.abs(v)

    def split_wq(slot, u, a, b):
        return sum(split(wq_f32[slot, 32 * i:32 * i + 32] * Q_SCALE, 16 * u + i) for i in range(a, b))

    def pivot_of(magnitudes):
        v = jnp.sum(magnitudes, axis=0, keepdims=True) * (PIVOT_RATIO / (32 * QUADS))
        return _shr(pltpu.bitcast(jnp.broadcast_to(v, (8, 128)), I32), 16) | 0x8000

    def encode(m, pivot, pos, bad, out):
        pivot = _pivot_bytes(pivot)
        for t in range(QUADS * m, QUADS * (m + 1)):
            h = _from_pivot(high[OWN, _quads(t)], low[OWN, _quads(t)], pivot)
            high[OWN, _quads(t)] = h
            signs = h & _bytes(0x80) if t % 8 == 0 else signs | _shr(h & _bytes(0x80), t % 8)
            if t % 8 == 7:
                code[OWN, pl.ds(SIGN_ROW[m] + t % QUADS - 7, 8)] = signs
            d = h & _bytes(0x7F)
            n = d + (_shr(d + _bytes(0x7C), 7) & _bytes(0x01)) + (_shr(_bytes(0x80) - d, 5) & _bytes(0x04))
            n0, n1, n2, n3 = n & 31, _shr(n, 8) & 31, _shr(n, 16) & 31, _shr(n, 24) & 31
            bits = _shr(zero + TOP_BIT, n3) | TOP_BIT
            bits = _shr(_shr(_shr(bits, n2) | TOP_BIT, n1) | TOP_BIT, (n0 - 1) & 31)
            length = (n0 + n1) + (n2 + n3)
            lo, hi = _window(t)
            if t and lo > _window(t - 1)[0]:
                pos = jnp.maximum(pos, 32 * lo)
                code[OWN, _stream_word(lo - 1)] = out.pop(lo - 1)
            bad = bad | (n & _bytes(0xE0)) | ((32 - length) & TOP_BIT)
            if _window(t + 1)[1] > hi or t % QUADS == QUADS - 1:
                bad = bad | ((32 * hi - 1 - pos) & TOP_BIT)
            word, shift = _shr(pos, 5), pos & 31
            head, rest = _shr(bits, shift), _shl(_shl(bits, 1), 31 - shift)
            for i in range(lo, hi + 1):
                v = jnp.where(word == i - 1, rest, 0) if i > lo else zero
                v = jnp.where(word == i, head, v) if i < hi else v
                out[i] = out[i] | v if i in out else v
            pos = pos + length
        return pos, bad, out

    def header_half(pivot, bad):
        bad = jnp.max(jnp.where(bad != 0, 1.0, 0.0), axis=0, keepdims=True)
        return jnp.where(jnp.max(bad, axis=1, keepdims=True) > 0.0, pivot[:1] & 0x7FFF, pivot[:1])

    def misfits(s):
        header = code[s, pl.ds(HEADER_ROW, 1)][0, 0]
        return (header & 0x8000) == 0, header >= 0

    def pivot_from(s, m):
        header = jnp.broadcast_to(code[s, pl.ds(HEADER_ROW, 1)], (8, 128))
        return _pivot_bytes((header & 0xFFFF if m == WQ else _shr(header, 16)) | 0x8000)

    def decode(m, positions):
        cache = {}

        def word(s, i):
            if (s, i) not in cache:
                cache[s, i] = (code[s, _stream_word(i)] if i < STREAM_WORDS
                               else _mirrored(word(s, 2 * STREAM_WORDS - 1 - i)))
            return cache[s, i]

        positions = dict(positions)
        for t in range(QUADS * m, QUADS * (m + 1)):
            lo, hi = _window(t)
            for s, pos in positions.items():
                if t and lo > _window(t - 1)[0]:
                    pos = jnp.maximum(pos, 32 * lo)
                a, b = word(s, lo), word(s, lo + 1)
                for i in range(lo + 1, hi):
                    past = pos >= 32 * i
                    a, b = jnp.where(past, word(s, i), a), jnp.where(past, word(s, i + 1), b)
                shift = pos & 31
                bits = _shl(a, shift) | _shr(_shr(b, 1), 31 - shift)
                z0 = lax.clz(bits)
                bits = _shl(_shl(bits, 1), z0)
                z1 = lax.clz(bits)
                bits = _shl(_shl(bits, 1), z1)
                z2 = lax.clz(bits)
                z3 = lax.clz(_shl(_shl(bits, 1), z2))
                positions[s] = (pos + 4 + z0) + (z1 + z2) + z3
                z = (z0 | _shl(z1, 8)) | (_shl(z2, 16) | _shl(z3, 24))
                short = _shr(_bytes(0x83) - z, 7) & _bytes(0x01)
                signs = code[s, pl.ds(SIGN_ROW[m] + t % QUADS // 8 * 8, 8)]
                signs = (_shl(signs, t % 8) if t % 8 else signs) & _bytes(0x80)
                high[s, _quads(t)] = ((z + short) & ~_shl(short, 2)) | signs
        return positions

    def unless_it_fit(s, m):
        @pl.when(misfit[s][m])
        def _():
            if s == FAR:
                arrived(far_plain[m])
            else:
                plain[m][s - LEFT].wait_recv()
                far_plain[m][s - LEFT].start()
            high[s, _quads(QUADS * m, QUADS)] = uncoded[s, _quads(QUADS * m, QUADS)]

    def weights(s, first, n, pivot=None):
        pivot = pivot or pivot_from(s, first // QUADS)
        out = []
        for t in range(first, first + n):
            l = low[s, _quads(t)]
            out += _interleave(l, _from_pivot(high[s, _quads(t)], l, pivot))
        return _halves(jnp.concatenate(out, axis=0))

    first_half = lax.broadcasted_iota(I32, (64, 128), 1) < 64
    tiles = [(b, j) for b in range(2) for j in range(2)]

    def loaded(*units):
        for unit in units:
            for copy in load_kv[unit]:
                copy.wait()

    def prepare(s, u):
        for b, j in tiles:
            k = kt_f32[s, u, b, :, 128 * j:128 * j + 128].T
            kb[s, u, b, j, 0:32] = _words(jnp.where(first_half, k[:64], k[64:]))
            kb[s, u, b, j, 32:64] = _words(jnp.where(first_half, k[64:], k[:64]))
            vb[s, u, b, j] = _words(vt_f32[s, u, b, :, 128 * j:128 * j + 128])

    def queries(s, u):
        return jnp.dot(_halves(xb[...]), weights(s, 16 * u, 16), preferred_element_type=F32)

    def diagonal(a, b):
        return jnp.concatenate([jnp.where(first_half, a, 0.0), jnp.where(first_half, 0.0, b)], 0).astype(BF16)

    def scores(s, u, q):
        out = []
        for b, j in tiles:
            r = 256 * b + 128 * j
            q0, q1 = q[r:r + 64], q[r + 64:r + 128]
            cross = jnp.concatenate([jnp.where(first_half, 0.0, q0), jnp.where(first_half, q1, 0.0)], 0)
            out.append([lax.dot_general(_halves(kb[s, u, b, j, 32 * i:32 * i + 32]), w, (((1,), (1,)), ((), ())),
                                        preferred_element_type=F32)
                        for i, w in enumerate((diagonal(q0, q1), cross.astype(BF16)))])
        return s, u, out

    def softmax(st):
        p = jnp.exp2(st - jnp.max(st, axis=0, keepdims=True))
        return p, 1.0 / jnp.sum(p, axis=0, keepdims=True)

    def values(s, u, sc):
        for (b, j), (s1, s2) in zip(tiles, sc):
            (p1, r1), (p2, r2) = softmax(s1), softmax(s2)
            c0 = jnp.dot(_halves(vb[s, u, b, j, 0:32]), diagonal(p1, p2), preferred_element_type=F32)
            c1 = jnp.dot(_halves(vb[s, u, b, j, 32:64]), diagonal(p2, p1), preferred_element_type=F32)
            c = jnp.concatenate([c0 * jnp.where(first_half[:1], r1, r2), c1 * jnp.where(first_half[:1], r2, r1)], 0)
            ctx[s, u, pl.ds(128 * b + 64 * j, 64)] = _words(c.T)

    def attend(s, u, previous=None):
        q = queries(s, u)
        if previous is not None:
            values(*previous)
        return scores(s, u, q)

    def projected(units, n, pivot=None):
        lhs = jnp.concatenate([_halves(ctx[s, u]) for s, u in units], axis=1)
        rhs = jnp.concatenate([weights(s, QUADS + 16 * u + 4 * n, 4, pivot) for s, u in units], axis=0)
        return [jnp.dot(lhs[256 * b:256 * b + 256], rhs, preferred_element_type=F32) for b in range(2)]

    def accumulate(units, columns):
        for n in columns:
            for b, y in enumerate(projected(units, n)):
                acc[b, :, 128 * n:128 * n + 128] += y

    magnitudes = 0.0
    for (a, b), copy in zip(spans, load_lead):
        if b == 16:
            load_other[0].wait()
            magnitudes += split_wq(1, 1 - lead, 0, 6)
            pl.when(even)(lambda: start((first_pair(1 - lead, 0, 1, 2), first_pair(1 - lead, 1, 5, 0))))
        copy.wait()
        magnitudes += split_wq(0, lead, a, b)
        first_pair(lead, a, b - a, 0).start()
    load_lead0.wait()
    magnitudes += split_wq(0, lead, 0, 1)
    pl.when(even)(lambda: first_pair(lead, 0, 1, 2).start())
    load_other[1].wait()
    magnitudes += split_wq(1, 1 - lead, 6, 16)
    pl.when(even)(lambda: first_pair(1 - lead, 6, 10, 0).start())
    pivot_q = pivot_of(magnitudes)
    pos, bad_q, out = encode(WQ, pivot_q, zero, zero, {})

    @pl.when(odd)
    def _():
        pl.semaphore_wait(ready, 1)
        start((first_pair(1 - lead, 0, 1, 2), first_pair(1 - lead, 1, 15, 0)))

    start(code_q1)
    load_wo.wait()
    pivot_o = pivot_of(sum(
        split(wo_f32[pl.ds(128 * u + 32 * i, 32), pl.ds(128 * n, 128)], QUADS + 16 * u + 4 * n + i)
        for u in range(2) for n in range(4) for i in range(4)))
    pos, bad_o, out = encode(WO, pivot_o, pos, bad_q, out)
    for i in range(min(out), STREAM_WORDS):
        code[OWN, _stream_word(i)] = out[i] | _mirrored(out[2 * STREAM_WORDS - 1 - i])
    bad_o = bad_o | ((64 * STREAM_WORDS - pos - pltpu.roll(pos, 4, 0)) & TOP_BIT)
    code[OWN, pl.ds(HEADER_ROW, 1)] = header_half(pivot_q, bad_q) | _shl(header_half(pivot_o, bad_o), 16)
    start(code_q2, code_o, low_q2, low_o1[0])
    misfit = {OWN: misfits(OWN)}
    for m in (WQ, WO):
        pl.when(misfit[OWN][m])(lambda: start(plain[m]))

    load_x.wait()
    for b in range(2):
        xb[128 * b:128 * b + 128] = _words(x_f32[b])
    q0, q1 = queries(OWN, 0), queries(OWN, 1)
    loaded((OWN, 0))
    prepare(OWN, 0)
    pending = scores(OWN, 0, q0)
    loaded((OWN, 1))
    prepare(OWN, 1)
    values(*pending)
    values(*scores(OWN, 1, q1))

    @pl.when(me == 0)
    def _():
        for u in range(2):
            unrounded(u).wait_recv()
            w = _words(early[u] * Q_SCALE)
            low[LEFT + u, _quads(16 * u)] = _interleave(w[:8], w[8:])[0]

    pl.when(me != 0)(lambda: arrived([first_pair(u, 0, 1, 2) for u in range(2)]))
    arrived([first_pair(u, 1, 15, 0) for u in range(2)], code_q1, code_q2)
    start(far_code_q, far_low_q, *low_o1[1:])
    misfit[LEFT], misfit[RIGHT] = misfits(LEFT), misfits(RIGHT)
    near = decode(WQ, {LEFT: zero, RIGHT: zero})
    for n in range(4):
        for b, y in enumerate(projected([(OWN, 0), (OWN, 1)], n)):
            acc[b, :, 128 * n:128 * n + 128] = y
    unless_it_fit(LEFT, WQ)
    unless_it_fit(RIGHT, WQ)

    arrived(code_o)
    loaded((LEFT, 0), (RIGHT, 1))
    start(far_code_o, *low_o2)
    decode(WO, {LEFT: near[LEFT]})
    prepare(LEFT, 0)
    pending = attend(LEFT, 0)
    prepare(RIGHT, 1)
    pending = attend(RIGHT, 1, pending)

    arrived(low_q2)
    loaded((LEFT, 1), (RIGHT, 0))
    decode(WO, {RIGHT: near[RIGHT]})
    prepare(LEFT, 1)
    pending = attend(LEFT, 1, pending)
    prepare(RIGHT, 0)
    pending = attend(RIGHT, 0, pending)
    unless_it_fit(LEFT, WO)
    unless_it_fit(RIGHT, WO)

    sooner, later = [(LEFT, 0), (RIGHT, 1)], [(LEFT, 1), (RIGHT, 0)]
    arrived(far_code_q, low_o1[0])
    loaded((FAR, 0), (FAR, 1))
    start(far_low_o[0])
    misfit[FAR] = misfits(FAR)
    far = decode(WQ, {FAR: zero})
    values(*pending)
    prepare(FAR, 0)
    prepare(FAR, 1)
    accumulate(sooner, [0])
    unless_it_fit(FAR, WQ)

    drained(code_q1, code_q2, code_o, low_q2, low_o1[0], [first_pair(u, 1, 15, 0) for u in range(2)])
    first_pair(1 - lead, 0, 1, 2).wait_send()
    pl.when(even)(lambda: first_pair(lead, 0, 1, 2).wait_send())
    pl.when(odd)(lambda: unrounded(lead).wait_send())
    arrived(far_low_q)
    pending = attend(FAR, 0)

    arrived(low_o1[1])
    start(*far_low_o[1:3])
    pending = attend(FAR, 1, pending)
    accumulate(sooner, [1])

    arrived(low_o1[2])
    start(far_low_o[3])
    arrived(far_code_o)
    decode(WO, far)
    values(*pending)
    accumulate(sooner, [2, 3])
    unless_it_fit(FAR, WO)

    arrived(low_o2[0])
    accumulate(later, [0, 1])

    drained(far_code_q, far_low_q, *low_o1[1:], far_code_o, low_o2[0])
    for m in (WQ, WO):
        pl.when(misfit[OWN][m])(lambda: drained(plain[m]))
        for s in (LEFT, RIGHT):
            pl.when(misfit[s][m])(far_plain[m][s - LEFT].wait_send)
    arrived(low_o2[1])
    pivot = pivot_from(FAR, WO)
    accumulate(later, [2, 3])

    for n in range(4):
        if n == 2:
            drained(low_o2[1], *far_low_o[:2])
        if n == 3:
            drained(*far_low_o[2:])
        arrived(far_low_o[n])
        columns = pl.ds(128 * n, 128)
        for b, y in enumerate(projected([(FAR, 0), (FAR, 1)], n, pivot)):
            o_ref[b, :, columns] = (y + acc[b, :, columns]).astype(o_ref.dtype)


def pallas_dist_sparse_attn_strided_htp_bs_b2_sq256_skv256_hq4_dh64_kernel(
    x: jax.Array,
    Wq: jax.Array,
    K_ext: jax.Array,
    V_ext: jax.Array,
    Wo: jax.Array,
):
    kt = jnp.transpose(K_ext, (0, 2, 3, 1)).reshape(8, 1024, 256)
    vt = jnp.transpose(V_ext, (0, 2, 3, 1)).reshape(8, 1024, 256)
    plane = pltpu.VMEM((4, 16 * QUADS, 128), I32)
    return pl.pallas_call(
        _body,
        out_shape=jax.ShapeDtypeStruct(x.shape, BF16),
        in_specs=[pl.BlockSpec(memory_space=pltpu.HBM)] * 5,
        out_specs=pl.BlockSpec(memory_space=pltpu.VMEM),
        scratch_shapes=[
            pltpu.VMEM((2, 256, 512), F32),
            pltpu.VMEM((2, 512, 128), F32),
            pltpu.VMEM((256, 512), F32),
            pltpu.VMEM((4, 2, 2, 128, 256), F32),
            pltpu.VMEM((4, 2, 2, 128, 256), F32),
            pltpu.VMEM((2, 32, 128), F32),
            plane, plane, plane,
            pltpu.VMEM((4, CODE_ROWS, 128), I32),
            pltpu.VMEM((256, 512), I32),
            pltpu.VMEM((4, 2, 2, 2, 64, 128), I32),
            pltpu.VMEM((4, 2, 2, 2, 64, 128), I32),
            pltpu.VMEM((4, 2, 256, 128), I32),
            pltpu.VMEM((2, 256, 512), F32),
            pltpu.SemaphoreType.DMA((26,)),
            pltpu.SemaphoreType.DMA((46,)),
            pltpu.SemaphoreType.DMA((46,)),
            pltpu.SemaphoreType.REGULAR,
        ],
        compiler_params=pltpu.CompilerParams(
            collective_id=0, disable_semaphore_checks=True, vmem_limit_bytes=32 * 1024 * 1024),
    )(x, Wq, kt, vt, Wo)
```

```python
import math

import jax
import jax.numpy as jnp
import numpy as np
from jax import lax
from jax.experimental import pallas as pl
from jax.experimental.pallas import tpu as pltpu

BF16, F32, I32 = jnp.bfloat16, jnp.float32, jnp.int32
MESH = pl.DeviceIdType.MESH
Q_SCALE = 0.125 * math.log2(math.e)
OWN, LEFT, RIGHT, FAR = 0, 1, 2, 3
WQ, WO = 0, 1

QUADS = 32
STREAM_WORDS = 15
PIVOT_RATIO = 10.8
SIGN_ROW, HEADER_ROW, CODE_ROWS = (0, 160), 112, 192


def _i32(v):
    return np.uint32(v).astype(np.int32)


def _bytes(b):
    return _i32(b * 0x01010101)


EVEN, ODD, TOP_BIT = _i32(0x00FF00FF), _i32(0xFF00FF00), _i32(0x80000000)


def _shl(v, n):
    return lax.shift_left(v, jnp.full_like(v, n) if isinstance(n, int) else n)


def _shr(v, n):
    return lax.shift_right_logical(v, jnp.full_like(v, n) if isinstance(n, int) else n)


def _words(v):
    return pltpu.bitcast(v.astype(BF16), I32)


def _halves(w):
    return pltpu.bitcast(w, BF16)


def _aligned(start, size, align):
    return pl.ds(start if isinstance(start, int) else pl.multiple_of(start, align), size)


def _quads(first, n=1):
    return _aligned(8 * first, 8 * n, 8)


def _stream_word(i):
    return pl.ds(32 + 8 * i if i < 10 else 40 + 8 * i, 8)


def _window(t):
    mean, dev = 6.7 * t, 1.9 * math.sqrt(t)
    return (max(math.floor((mean - dev) / 32), 0),
            math.floor((mean + 5.3 * dev + (10 if t else 0)) / 32) + 1)


def _mirrored(v):
    v = pltpu.roll(v, 4, 0)
    for k, mask in ((1, 0x55555555), (2, 0x33333333), (4, 0x0F0F0F0F), (8, 0x00FF00FF)):
        v = (_shr(v, k) & mask) | _shl(v & mask, k)
    return _shr(v, 16) | _shl(v, 16)


def _interleave(a, b):
    return (a & EVEN) | (_shl(b, 8) & ODD), (_shr(a, 8) & EVEN) | (b & ODD)


def _pivot_bytes(pivot):
    def spread(v):
        v = v | _shl(v, 8)
        return v | _shl(v, 16)
    return spread(_shr(pivot, 8)), spread(127 - _shr(pivot & 0xFF, 1))


def _from_pivot(high, low, pivot_bytes):
    borrow = _shr((_shr(low, 1) & _bytes(0x7F)) + pivot_bytes[1], 7) & _bytes(0x01)
    return pivot_bytes[0] - high - borrow


def _body(x_hbm, wq_hbm, kt_hbm, vt_hbm, wo_hbm, o_ref,
          x_f32, wq_f32, wo_f32, kt_f32, vt_f32, low, high, uncoded, code, xb, kb, vb, ctx, acc,
          load_sem, send_sem, recv_sem, ready):
    me = lax.axis_index("i")
    left, right = (me + 3) & 3, (me + 1) & 3
    odd = (me & 1) == 1
    even = jnp.logical_not(odd)
    barrier = pltpu.get_barrier_semaphore()

    def remote(src, dst, k, to):
        return pltpu.make_async_remote_copy(src, dst, send_sem.at[k], recv_sem.at[k],
                                            device_id=(to,), device_id_type=MESH)

    def low_q1(u, a=0, b=16):
        rows = _quads(16 * u + a, b - a)
        return remote(low.at[OWN, rows], low.at[LEFT + u, rows], u, (me + 1 + 2 * u) & 3)

    free_sems = iter(range(2, send_sem.shape[0]))

    def mine(buf, rows_r, rows_l, dst=None):
        dst = buf if dst is None else dst
        return (remote(buf.at[OWN, rows_r], dst.at[LEFT, rows_r], next(free_sems), right),
                remote(buf.at[OWN, rows_l], dst.at[RIGHT, rows_l], next(free_sems), left))

    def onward(buf, rows_r, rows_l):
        return (remote(buf.at[LEFT, rows_r], buf.at[FAR, rows_r], next(free_sems), right),
                remote(buf.at[RIGHT, rows_l], buf.at[FAR, rows_l], next(free_sems), left))

    code_q1 = mine(code, pl.ds(0, 80), pl.ds(0, 80))
    code_q2 = mine(code, pl.ds(80, 33), pl.ds(80, 33))
    code_o = mine(code, pl.ds(120, 72), pl.ds(120, 72))
    low_q2 = mine(low, _quads(16, 16), _quads(0, 16))
    low_o1 = [mine(low, _quads(32 + a, n), _quads(48 + a, n)) for a, n in ((0, 4), (4, 8), (12, 4))]
    low_o2 = [mine(low, _quads(48 + a, 8), _quads(32 + a, 8)) for a in (0, 8)]
    far_code_q = onward(code, pl.ds(0, 56), pl.ds(56, 57))
    far_code_o = onward(code, pl.ds(120, 40), pl.ds(160, 32))
    far_low_q = onward(low, _quads(0, 16), _quads(16, 16))
    far_low_o = [onward(low, _quads(32 + 4 * n, 4), _quads(48 + 4 * n, 4)) for n in range(4)]
    plain = [mine(high, _quads(QUADS * m, QUADS), _quads(QUADS * m, QUADS), uncoded) for m in (WQ, WO)]
    far_plain = [onward(uncoded, _quads(QUADS * m, 16), _quads(QUADS * m + 16, 16)) for m in (WQ, WO)]

    def start(*pairs):
        for pair in pairs:
            for copy in pair:
                copy.start()

    def arrived(*pairs):
        for pair in pairs:
            for copy in pair:
                copy.wait_recv()

    def drained(*pairs):
        for pair in pairs:
            for copy in pair:
                copy.wait_send()

    lead = jnp.where(me == 1, 1, 0)
    spans = ((0, 1), (1, 2), (2, 4), (4, 8), (8, 16))
    free_loads = iter(range(load_sem.shape[0]))

    def load(src, dst):
        return pltpu.make_async_copy(src, dst, load_sem.at[next(free_loads)])

    def load_wq(slot, u, a, b):
        rows = pl.ds(32 * a, 32 * (b - a))
        return load(wq_hbm.at[rows, _aligned(128 * u, 128, 128)], wq_f32.at[slot, rows])

    load_lead = [load_wq(0, lead, a, b) for a, b in spans]
    load_other = [load_wq(1, 1 - lead, 0, 6), load_wq(1, 1 - lead, 6, 16)]
    load_wo, load_x = load(wo_hbm, wo_f32), load(x_hbm, x_f32)
    load_lead[0].start()

    @pl.when(me != 2)
    def _():
        for to in (left, right):
            pl.semaphore_signal(barrier, 1, device_id=(to,), device_id_type=MESH)

    for copy in (*load_lead[1:-1], load_other[0], load_lead[-1], load_other[1], load_wo, load_x):
        copy.start()
    owner = (me, left, right, (me + 2) & 3)
    load_kv = {}
    for s, u in ((OWN, 0), (OWN, 1), (LEFT, 0), (RIGHT, 1), (LEFT, 1), (RIGHT, 0), (FAR, 0), (FAR, 1)):
        part = (pl.ds(2 * me, 2), _aligned(256 * owner[s] + 128 * u, 128, 128))
        load_kv[s, u] = (load(kt_hbm.at[part], kt_f32.at[s, u]), load(vt_hbm.at[part], vt_f32.at[s, u]))
        start(load_kv[s, u])

    pl.when(odd)(lambda: pl.semaphore_wait(barrier, 1))

    @pl.when(even)
    def _():
        pl.semaphore_wait(barrier, 2)

        @pl.when(me == 2)
        def _():
            for to in (left, right):
                pl.semaphore_signal(ready, 1, device_id=(to,), device_id_type=MESH)

    zero = jnp.zeros((8, 128), I32)

    def split(v, t):
        w = _words(v)
        low[OWN, _quads(t)], high[OWN, _quads(t)] = _interleave(w[:8], w[8:])
        return jnp.abs(v)

    def split_wq(slot, u, a, b):
        return sum(split(wq_f32[slot, 32 * i:32 * i + 32] * Q_SCALE, 16 * u + i) for i in range(a, b))

    def pivot_of(magnitudes):
        v = jnp.sum(magnitudes, axis=0, keepdims=True) * (PIVOT_RATIO / (32 * QUADS))
        return _shr(pltpu.bitcast(jnp.broadcast_to(v, (8, 128)), I32), 16) | 0x8000

    def encode(m, pivot, pos, bad, out):
        pivot = _pivot_bytes(pivot)
        for t in range(QUADS * m, QUADS * (m + 1)):
            h = _from_pivot(high[OWN, _quads(t)], low[OWN, _quads(t)], pivot)
            high[OWN, _quads(t)] = h
            signs = h & _bytes(0x80) if t % 8 == 0 else signs | _shr(h & _bytes(0x80), t % 8)
            if t % 8 == 7:
                code[OWN, pl.ds(SIGN_ROW[m] + t % QUADS - 7, 8)] = signs
            d = h & _bytes(0x7F)
            n = d + (_shr(d + _bytes(0x7C), 7) & _bytes(0x01)) + (_shr(_bytes(0x80) - d, 5) & _bytes(0x04))
            n0, n1, n2, n3 = n & 31, _shr(n, 8) & 31, _shr(n, 16) & 31, _shr(n, 24) & 31
            bits = _shr(zero + TOP_BIT, n3) | TOP_BIT
            bits = _shr(_shr(_shr(bits, n2) | TOP_BIT, n1) | TOP_BIT, (n0 - 1) & 31)
            length = (n0 + n1) + (n2 + n3)
            lo, hi = _window(t)
            if t and lo > _window(t - 1)[0]:
                pos = jnp.maximum(pos, 32 * lo)
                code[OWN, _stream_word(lo - 1)] = out.pop(lo - 1)
            bad = bad | (n & _bytes(0xE0)) | ((32 - length) & TOP_BIT)
            if _window(t + 1)[1] > hi or t % QUADS == QUADS - 1:
                bad = bad | ((32 * hi - 1 - pos) & TOP_BIT)
            word, shift = _shr(pos, 5), pos & 31
            head, rest = _shr(bits, shift), _shl(_shl(bits, 1), 31 - shift)
            for i in range(lo, hi + 1):
                v = jnp.where(word == i - 1, rest, 0) if i > lo else zero
                v = jnp.where(word == i, head, v) if i < hi else v
                out[i] = out[i] | v if i in out else v
            pos = pos + length
        return pos, bad, out

    def header_half(pivot, bad):
        bad = jnp.max(jnp.where(bad != 0, 1.0, 0.0), axis=0, keepdims=True)
        return jnp.where(jnp.max(bad, axis=1, keepdims=True) > 0.0, pivot[:1] & 0x7FFF, pivot[:1])

    def misfits(s):
        header = code[s, pl.ds(HEADER_ROW, 1)][0, 0]
        return (header & 0x8000) == 0, header >= 0

    def pivot_from(s, m):
        header = jnp.broadcast_to(code[s, pl.ds(HEADER_ROW, 1)], (8, 128))
        return _pivot_bytes((header & 0xFFFF if m == WQ else _shr(header, 16)) | 0x8000)

    def decode(m, positions):
        cache = {}

        def word(s, i):
            if (s, i) not in cache:
                cache[s, i] = (code[s, _stream_word(i)] if i < STREAM_WORDS
                               else _mirrored(word(s, 2 * STREAM_WORDS - 1 - i)))
            return cache[s, i]

        positions = dict(positions)
        for t in range(QUADS * m, QUADS * (m + 1)):
            lo, hi = _window(t)
            for s, pos in positions.items():
                if t and lo > _window(t - 1)[0]:
                    pos = jnp.maximum(pos, 32 * lo)
                a, b = word(s, lo), word(s, lo + 1)
                for i in range(lo + 1, hi):
                    past = pos >= 32 * i
                    a, b = jnp.where(past, word(s, i), a), jnp.where(past, word(s, i + 1), b)
                shift = pos & 31
                bits = _shl(a, shift) | _shr(_shr(b, 1), 31 - shift)
                z0 = lax.clz(bits)
                bits = _shl(_shl(bits, 1), z0)
                z1 = lax.clz(bits)
                bits = _shl(_shl(bits, 1), z1)
                z2 = lax.clz(bits)
                z3 = lax.clz(_shl(_shl(bits, 1), z2))
                positions[s] = (pos + 4 + z0) + (z1 + z2) + z3
                z = (z0 | _shl(z1, 8)) | (_shl(z2, 16) | _shl(z3, 24))
                short = _shr(_bytes(0x83) - z, 7) & _bytes(0x01)
                signs = code[s, pl.ds(SIGN_ROW[m] + t % QUADS // 8 * 8, 8)]
                signs = (_shl(signs, t % 8) if t % 8 else signs) & _bytes(0x80)
                high[s, _quads(t)] = ((z + short) & ~_shl(short, 2)) | signs
        return positions

    def unless_it_fit(s, m):
        @pl.when(misfit[s][m])
        def _():
            if s == FAR:
                arrived(far_plain[m])
            else:
                plain[m][s - LEFT].wait_recv()
                far_plain[m][s - LEFT].start()
            high[s, _quads(QUADS * m, QUADS)] = uncoded[s, _quads(QUADS * m, QUADS)]

    def weights(s, first, n, pivot=None):
        pivot = pivot or pivot_from(s, first // QUADS)
        out = []
        for t in range(first, first + n):
            l = low[s, _quads(t)]
            out += _interleave(l, _from_pivot(high[s, _quads(t)], l, pivot))
        return _halves(jnp.concatenate(out, axis=0))

    first_half = lax.broadcasted_iota(I32, (64, 128), 1) < 64
    tiles = [(b, j) for b in range(2) for j in range(2)]

    def loaded(*units):
        for unit in units:
            for copy in load_kv[unit]:
                copy.wait()

    def prepare(s, u):
        for b, j in tiles:
            k = kt_f32[s, u, b, :, 128 * j:128 * j + 128].T
            kb[s, u, b, j, 0:32] = _words(jnp.where(first_half, k[:64], k[64:]))
            kb[s, u, b, j, 32:64] = _words(jnp.where(first_half, k[64:], k[:64]))
            vb[s, u, b, j] = _words(vt_f32[s, u, b, :, 128 * j:128 * j + 128])

    def queries(s, u):
        return jnp.dot(_halves(xb[...]), weights(s, 16 * u, 16), preferred_element_type=F32)

    def diagonal(a, b):
        return jnp.concatenate([jnp.where(first_half, a, 0.0), jnp.where(first_half, 0.0, b)], 0).astype(BF16)

    def scores(s, u, q):
        out = []
        for b, j in tiles:
            r = 256 * b + 128 * j
            q0, q1 = q[r:r + 64], q[r + 64:r + 128]
            cross = jnp.concatenate([jnp.where(first_half, 0.0, q0), jnp.where(first_half, q1, 0.0)], 0)
            out.append([lax.dot_general(_halves(kb[s, u, b, j, 32 * i:32 * i + 32]), w, (((1,), (1,)), ((), ())),
                                        preferred_element_type=F32)
                        for i, w in enumerate((diagonal(q0, q1), cross.astype(BF16)))])
        return s, u, out

    def softmax(st):
        p = jnp.exp2(st - jnp.max(st, axis=0, keepdims=True))
        return p, 1.0 / jnp.sum(p, axis=0, keepdims=True)

    def values(s, u, sc):
        for (b, j), (s1, s2) in zip(tiles, sc):
            (p1, r1), (p2, r2) = softmax(s1), softmax(s2)
            c0 = jnp.dot(_halves(vb[s, u, b, j, 0:32]), diagonal(p1, p2), preferred_element_type=F32)
            c1 = jnp.dot(_halves(vb[s, u, b, j, 32:64]), diagonal(p2, p1), preferred_element_type=F32)
            c = jnp.concatenate([c0 * jnp.where(first_half[:1], r1, r2), c1 * jnp.where(first_half[:1], r2, r1)], 0)
            ctx[s, u, pl.ds(128 * b + 64 * j, 64)] = _words(c.T)

    def attend(s, u, previous=None):
        q = queries(s, u)
        if previous is not None:
            values(*previous)
        return scores(s, u, q)

    def projected(units, n, pivot=None):
        lhs = jnp.concatenate([_halves(ctx[s, u]) for s, u in units], axis=1)
        rhs = jnp.concatenate([weights(s, QUADS + 16 * u + 4 * n, 4, pivot) for s, u in units], axis=0)
        return [jnp.dot(lhs[256 * b:256 * b + 256], rhs, preferred_element_type=F32) for b in range(2)]

    def accumulate(units, columns):
        for n in columns:
            for b, y in enumerate(projected(units, n)):
                acc[b, :, 128 * n:128 * n + 128] += y

    magnitudes = 0.0
    for (a, b), copy in zip(spans, load_lead):
        if b == 16:
            load_other[0].wait()
            magnitudes += split_wq(1, 1 - lead, 0, 6)
            pl.when(even)(lambda: low_q1(1 - lead, 0, 6).start())
        copy.wait()
        magnitudes += split_wq(0, lead, a, b)
        low_q1(lead, a, b).start()
    load_other[1].wait()
    magnitudes += split_wq(1, 1 - lead, 6, 16)
    pl.when(even)(lambda: low_q1(1 - lead, 6, 16).start())
    pivot_q = pivot_of(magnitudes)
    pos, bad_q, out = encode(WQ, pivot_q, zero, zero, {})

    @pl.when(odd)
    def _():
        pl.semaphore_wait(ready, 1)
        low_q1(1 - lead).start()

    start(code_q1)
    load_wo.wait()
    pivot_o = pivot_of(sum(
        split(wo_f32[pl.ds(128 * u + 32 * i, 32), pl.ds(128 * n, 128)], QUADS + 16 * u + 4 * n + i)
        for u in range(2) for n in range(4) for i in range(4)))
    pos, bad_o, out = encode(WO, pivot_o, pos, bad_q, out)
    for i in range(min(out), STREAM_WORDS):
        code[OWN, _stream_word(i)] = out[i] | _mirrored(out[2 * STREAM_WORDS - 1 - i])
    bad_o = bad_o | ((64 * STREAM_WORDS - pos - pltpu.roll(pos, 4, 0)) & TOP_BIT)
    code[OWN, pl.ds(HEADER_ROW, 1)] = header_half(pivot_q, bad_q) | _shl(header_half(pivot_o, bad_o), 16)
    start(code_q2, code_o, low_q2, low_o1[0])
    misfit = {OWN: misfits(OWN)}
    for m in (WQ, WO):
        pl.when(misfit[OWN][m])(lambda: start(plain[m]))

    load_x.wait()
    for b in range(2):
        xb[128 * b:128 * b + 128] = _words(x_f32[b])
    q0, q1 = queries(OWN, 0), queries(OWN, 1)
    loaded((OWN, 0))
    prepare(OWN, 0)
    pending = scores(OWN, 0, q0)
    loaded((OWN, 1))
    prepare(OWN, 1)
    values(*pending)
    values(*scores(OWN, 1, q1))

    arrived((low_q1(0), low_q1(1)), code_q1, code_q2)
    start(far_code_q, far_low_q, *low_o1[1:])
    misfit[LEFT], misfit[RIGHT] = misfits(LEFT), misfits(RIGHT)
    near = decode(WQ, {LEFT: zero, RIGHT: zero})
    for n in range(4):
        for b, y in enumerate(projected([(OWN, 0), (OWN, 1)], n)):
            acc[b, :, 128 * n:128 * n + 128] = y
    unless_it_fit(LEFT, WQ)
    unless_it_fit(RIGHT, WQ)

    arrived(code_o)
    loaded((LEFT, 0), (RIGHT, 1))
    start(far_code_o, *low_o2)
    decode(WO, {LEFT: near[LEFT]})
    prepare(LEFT, 0)
    pending = attend(LEFT, 0)
    prepare(RIGHT, 1)
    pending = attend(RIGHT, 1, pending)

    arrived(low_q2)
    loaded((LEFT, 1), (RIGHT, 0))
    decode(WO, {RIGHT: near[RIGHT]})
    prepare(LEFT, 1)
    pending = attend(LEFT, 1, pending)
    prepare(RIGHT, 0)
    pending = attend(RIGHT, 0, pending)
    unless_it_fit(LEFT, WO)
    unless_it_fit(RIGHT, WO)

    sooner, later = [(LEFT, 0), (RIGHT, 1)], [(LEFT, 1), (RIGHT, 0)]
    arrived(far_code_q, low_o1[0])
    loaded((FAR, 0), (FAR, 1))
    start(far_low_o[0])
    misfit[FAR] = misfits(FAR)
    far = decode(WQ, {FAR: zero})
    values(*pending)
    prepare(FAR, 0)
    prepare(FAR, 1)
    accumulate(sooner, [0])
    unless_it_fit(FAR, WQ)

    drained((low_q1(0), low_q1(1)), code_q1, code_q2, code_o, low_q2, low_o1[0])
    arrived(far_low_q)
    pending = attend(FAR, 0)

    arrived(low_o1[1])
    start(*far_low_o[1:3])
    pending = attend(FAR, 1, pending)
    accumulate(sooner, [1])

    arrived(low_o1[2])
    start(far_low_o[3])
    arrived(far_code_o)
    decode(WO, far)
    values(*pending)
    accumulate(sooner, [2, 3])
    unless_it_fit(FAR, WO)

    arrived(low_o2[0])
    accumulate(later, [0, 1])

    drained(far_code_q, far_low_q, *low_o1[1:], far_code_o, low_o2[0])
    for m in (WQ, WO):
        pl.when(misfit[OWN][m])(lambda: drained(plain[m]))
        for s in (LEFT, RIGHT):
            pl.when(misfit[s][m])(far_plain[m][s - LEFT].wait_send)
    arrived(low_o2[1])
    pivot = pivot_from(FAR, WO)
    accumulate(later, [2, 3])

    for n in range(4):
        if n == 2:
            drained(low_o2[1], *far_low_o[:2])
        if n == 3:
            drained(*far_low_o[2:])
        arrived(far_low_o[n])
        columns = pl.ds(128 * n, 128)
        for b, y in enumerate(projected([(FAR, 0), (FAR, 1)], n, pivot)):
            o_ref[b, :, columns] = (y + acc[b, :, columns]).astype(o_ref.dtype)


def pallas_dist_sparse_attn_strided_htp_bs_b2_sq256_skv256_hq4_dh64_kernel(
    x: jax.Array,
    Wq: jax.Array,
    K_ext: jax.Array,
    V_ext: jax.Array,
    Wo: jax.Array,
):
    kt = jnp.transpose(K_ext, (0, 2, 3, 1)).reshape(8, 1024, 256)
    vt = jnp.transpose(V_ext, (0, 2, 3, 1)).reshape(8, 1024, 256)
    plane = pltpu.VMEM((4, 16 * QUADS, 128), I32)
    return pl.pallas_call(
        _body,
        out_shape=jax.ShapeDtypeStruct(x.shape, BF16),
        in_specs=[pl.BlockSpec(memory_space=pltpu.HBM)] * 5,
        out_specs=pl.BlockSpec(memory_space=pltpu.VMEM),
        scratch_shapes=[
            pltpu.VMEM((2, 256, 512), F32),
            pltpu.VMEM((2, 512, 128), F32),
            pltpu.VMEM((256, 512), F32),
            pltpu.VMEM((4, 2, 2, 128, 256), F32),
            pltpu.VMEM((4, 2, 2, 128, 256), F32),
            plane, plane, plane,
            pltpu.VMEM((4, CODE_ROWS, 128), I32),
            pltpu.VMEM((256, 512), I32),
            pltpu.VMEM((4, 2, 2, 2, 64, 128), I32),
            pltpu.VMEM((4, 2, 2, 2, 64, 128), I32),
            pltpu.VMEM((4, 2, 256, 128), I32),
            pltpu.VMEM((2, 256, 512), F32),
            pltpu.SemaphoreType.DMA((25,)),
            pltpu.SemaphoreType.DMA((42,)),
            pltpu.SemaphoreType.DMA((42,)),
            pltpu.SemaphoreType.REGULAR,
        ],
        compiler_params=pltpu.CompilerParams(
            collective_id=0, disable_semaphore_checks=True, vmem_limit_bytes=32 * 1024 * 1024),
    )(x, Wq, kt, vt, Wo)
```
